```python
import numpy as np

kernel_name = "dist_sum_ax0_shard0_i_m1536_n768"

def setup_inputs():
    return {"x": np.random.randn(6144, 768).astype(np.float32)}

def reference(x: np.ndarray) -> np.ndarray:
    return np.sum(x, axis=0, keepdims=True)
```

```python
import jax
import jax.numpy as jnp
from jax import lax
from jax.experimental import pallas as pl
from jax.experimental.pallas import tpu as pltpu

N_DEV = 4
SUBLANES = 8
CHUNK_ROWS = (192, 192, 192, 192, 192, 192, 192, 192)
PEER_ORDER = (2, 1, 3)


def pallas_dist_sum_ax0_shard0_i_m1536_n768_kernel(
x: jax.Array,
):
    m, n = x.shape
    assert sum(CHUNK_ROWS) == m
    n_chunks = len(CHUNK_ROWS)
    offsets = [sum(CHUNK_ROWS[:c]) for c in range(n_chunks)]

    def kernel_body(x_ref, out_ref, xbuf, comm_ref, load_sems, send_sems,
                    recv_sems):
        me = lax.axis_index("i")

        loads = []
        for c in range(n_chunks):
            rows = pl.ds(offsets[c], CHUNK_ROWS[c])
            cp = pltpu.make_async_copy(
                x_ref.at[rows], xbuf.at[rows], load_sems.at[c])
            cp.start()
            loads.append(cp)

        barrier_sem = pltpu.get_barrier_semaphore()
        for d in range(1, N_DEV):
            pl.semaphore_signal(
                barrier_sem, inc=1, device_id=((me + d) % N_DEV,),
                device_id_type=pl.DeviceIdType.MESH)

        rdmas = []
        for d in PEER_ORDER:
            rdmas.append(pltpu.make_async_remote_copy(
                src_ref=comm_ref.at[0], dst_ref=comm_ref.at[d],
                send_sem=send_sems.at[d - 1], recv_sem=recv_sems.at[d - 1],
                device_id=((me + d) % N_DEV,),
                device_id_type=pl.DeviceIdType.MESH))

        acc = jnp.zeros((SUBLANES, n), jnp.float32)
        for c in range(n_chunks):
            if c == n_chunks - 1:
                pl.semaphore_wait(barrier_sem, N_DEV - 1)
            loads[c].wait()
            blk = xbuf[pl.ds(offsets[c], CHUNK_ROWS[c]), :]
            acc = acc + jnp.sum(
                blk.reshape(CHUNK_ROWS[c] // SUBLANES, SUBLANES, n), axis=0)
        part = jnp.sum(acc, axis=0, keepdims=True)

        comm_ref[0] = part
        for r in rdmas:
            r.start()
        for r in rdmas:
            r.wait_recv()
        out_ref[...] = (part + comm_ref[1]) + (comm_ref[2] + comm_ref[3])
        for r in rdmas:
            r.wait_send()

    return pl.pallas_call(
        kernel_body,
        out_shape=jax.ShapeDtypeStruct((1, n), x.dtype),
        in_specs=[pl.BlockSpec(memory_space=pl.ANY)],
        out_specs=pl.BlockSpec(memory_space=pltpu.VMEM),
        scratch_shapes=[
            pltpu.VMEM((m, n), jnp.float32),
            pltpu.VMEM((N_DEV, 1, n), jnp.float32),
            pltpu.SemaphoreType.DMA((n_chunks,)),
            pltpu.SemaphoreType.DMA((N_DEV - 1,)),
            pltpu.SemaphoreType.DMA((N_DEV - 1,)),
        ],
        compiler_params=pltpu.CompilerParams(collective_id=0),
    )(x)
```

```python
import jax
import jax.numpy as jnp
from jax import lax
from jax.experimental import pallas as pl
from jax.experimental.pallas import tpu as pltpu

N_DEV = 4
SUBLANES = 8
LANES = 128
CHUNK_ROWS = (192, 192, 192, 192, 192, 192, 192, 64)
SPLIT_ROWS = 128
DIAGONAL = 2
NEIGHBOURS = (1, 3)


def _tree_sum(vals):
    while len(vals) > 1:
        nxt = [vals[i] + vals[i + 1] for i in range(0, len(vals) - 1, 2)]
        if len(vals) % 2:
            nxt.append(vals[-1])
        vals = nxt
    return vals[0]


def _fold_rows(blk):
    r, c = blk.shape
    return jnp.sum(blk.reshape(r // SUBLANES, SUBLANES, c), axis=0)


def pallas_dist_sum_ax0_shard0_i_m1536_n768_kernel(
x: jax.Array,
):
    m, n = x.shape
    n_chunks = len(CHUNK_ROWS)
    offsets = [sum(CHUNK_ROWS[:c]) for c in range(n_chunks)]
    split_off = sum(CHUNK_ROWS)
    assert split_off + SPLIT_ROWS == m
    n_head, n_tail = n - LANES, LANES

    def kernel_body(x_ref, out_ref, xbuf, send_head, send_tail, recv_head,
                    recv_tail, load_sems, send_sems, recv_sems):
        me = lax.axis_index("i")

        def start_load(idx, rows, cols):
            cp = pltpu.make_async_copy(
                x_ref.at[rows, cols], xbuf.at[rows, cols], load_sems.at[idx])
            cp.start()
            return cp

        split_rows = pl.ds(split_off, SPLIT_ROWS)
        head_cols, tail_cols = pl.ds(0, n_head), pl.ds(n_head, n_tail)
        loads = [
            start_load(c, pl.ds(offsets[c], CHUNK_ROWS[c]), pl.ds(0, n))
            for c in range(n_chunks)
        ]
        head_load = start_load(n_chunks, split_rows, head_cols)
        tail_load = start_load(n_chunks + 1, split_rows, tail_cols)

        barrier_sem = pltpu.get_barrier_semaphore()
        for d in range(1, N_DEV):
            pl.semaphore_signal(
                barrier_sem, inc=1, device_id=((me + d) % N_DEV,),
                device_id_type=pl.DeviceIdType.MESH)

        def remote(src, dst, d, sem):
            return pltpu.make_async_remote_copy(
                src_ref=src, dst_ref=dst.at[d - 1],
                send_sem=send_sems.at[sem], recv_sem=recv_sems.at[sem],
                device_id=((me + d) % N_DEV,),
                device_id_type=pl.DeviceIdType.MESH)

        head_rdma = {d: remote(send_head, recv_head, d, d - 1)
                     for d in range(1, N_DEV)}
        tail_rdma = {d: remote(send_tail, recv_tail, d, N_DEV - 1 + d - 1)
                     for d in range(1, N_DEV)}

        acc = jnp.zeros((SUBLANES, n), jnp.float32)
        for c in range(n_chunks):
            if c == n_chunks - 1:
                pl.semaphore_wait(barrier_sem, N_DEV - 1)
            loads[c].wait()
            acc = acc + _fold_rows(xbuf[pl.ds(offsets[c], CHUNK_ROWS[c]), :])

        head_load.wait()
        acc_head = acc[:, :n_head] + _fold_rows(xbuf[split_rows, head_cols])
        send_head[...] = jnp.sum(acc_head, axis=0, keepdims=True)
        head_rdma[DIAGONAL].start()

        tail_load.wait()
        acc_tail = _tree_sum(
            [xbuf[pl.ds(split_off + SUBLANES * i, SUBLANES), tail_cols]
             for i in range(SPLIT_ROWS // SUBLANES)] + [acc[:, n_head:]])
        send_tail[...] = jnp.sum(acc_tail, axis=0, keepdims=True)
        tail_rdma[DIAGONAL].start()
        for d in NEIGHBOURS:
            head_rdma[d].start()
            tail_rdma[d].start()

        res_head = send_head[...]
        res_tail = send_tail[...]
        for d in NEIGHBOURS:
            head_rdma[d].wait_recv()
            res_head = res_head + recv_head[d - 1]
            tail_rdma[d].wait_recv()
            res_tail = res_tail + recv_tail[d - 1]
        for d in range(1, N_DEV):
            head_rdma[d].wait_send()
            tail_rdma[d].wait_send()
        head_rdma[DIAGONAL].wait_recv()
        out_ref[:, head_cols] = res_head + recv_head[DIAGONAL - 1]
        tail_rdma[DIAGONAL].wait_recv()
        out_ref[:, tail_cols] = res_tail + recv_tail[DIAGONAL - 1]

    return pl.pallas_call(
        kernel_body,
        out_shape=jax.ShapeDtypeStruct((1, n), x.dtype),
        in_specs=[pl.BlockSpec(memory_space=pl.ANY)],
        out_specs=pl.BlockSpec(memory_space=pltpu.VMEM),
        scratch_shapes=[
            pltpu.VMEM((m, n), jnp.float32),
            pltpu.VMEM((1, n_head), jnp.float32),
            pltpu.VMEM((1, n_tail), jnp.float32),
            pltpu.VMEM((N_DEV - 1, 1, n_head), jnp.float32),
            pltpu.VMEM((N_DEV - 1, 1, n_tail), jnp.float32),
            pltpu.SemaphoreType.DMA((n_chunks + 2,)),
            pltpu.SemaphoreType.DMA((2 * (N_DEV - 1),)),
            pltpu.SemaphoreType.DMA((2 * (N_DEV - 1),)),
        ],
        compiler_params=pltpu.CompilerParams(
            collective_id=0, disable_semaphore_checks=True),
    )(x)
```
